```python
import numpy as np

kernel_name = "dist_moe_shared_ep_outshard_n512_d256_e2_h512"

def setup_inputs():
    x = np.random.randn(512, 256).astype(np.float32)
    router_W = np.random.randn(256, 8).astype(np.float32) * 0.1
    scores64 = x.astype(np.float64) @ router_W.astype(np.float64)
    route_idx = np.argsort(-scores64, axis=-1)[:, :1].astype(np.int32)
    expert_W = np.random.randn(8, 256, 512).astype(np.float32) * 0.02
    shared_W = np.random.randn(256, 512).astype(np.float32) * 0.02
    return {"x": x, "router_W": router_W, "route_idx": route_idx, "expert_W": expert_W, "shared_W": shared_W}

def reference(x, router_W, route_idx, expert_W, shared_W):
    scores = x @ router_W
    s_max = scores.max(axis=-1, keepdims=True)
    probs = np.exp(scores - s_max)
    probs = probs / probs.sum(axis=-1, keepdims=True)
    shared = x @ shared_W
    out = np.zeros((512, 512), dtype=np.float32)
    for i in range(512):
        e = int(route_idx[i, 0])
        out[i] = shared[i] + probs[i, e] * (x[i] @ expert_W[e])
    return out
```

```python
import functools, contextlib
import jax
import jax.numpy as jnp
from jax import lax
from jax.experimental import pallas as pl
from jax.experimental.pallas import tpu as pltpu

NDEV = 4
NTOK = 512
BLK = NTOK // NDEV
D = 256
H = 512
NE = 8
EL = 2
NCH = 4
CW = H // NCH
G = 16
NG = BLK // G
MESH = pl.DeviceIdType.MESH
bf16, f32, i32, u32 = jnp.bfloat16, jnp.float32, jnp.int32, jnp.uint32

SCOPES = False
NOSEMCHK = 0
NOBOUNDS = 0
STAGES = [tuple(int(a) for a in s.split("-")) for s in '0-0,1-1,2-2,3-3'.split(",")]

def scope(name):
    return jax.named_scope(name) if SCOPES else contextlib.nullcontext()

def _dot(a, b):
    return jnp.dot(a, b, preferred_element_type=f32)

def _pack(v):
    w = pltpu.bitcast(v, u32)
    return w.reshape(w.shape[0] // 8, 8, w.shape[1])

def _unpack(w):
    return pltpu.bitcast(w.reshape(w.shape[0] * 8, w.shape[2]), bf16)


def _body(x_hbm, rw_hbm, idx_hbm, ew_hbm, sw_hbm, out_ref,
          idx_v, rw_v, x_v, w_v, sw_v, lhs_v, send_v, recv_v, own_v, pt_v,
          ld_sem, send_sem, recv_sem):
    me = lax.axis_index("i")
    odd = (me & 1) == 1
    even = jnp.logical_not(odd)
    first = me == 0
    late = jnp.logical_not(first)
    koff = [0, jnp.where(odd, (-me) & 3, 2), jnp.where(odd, 2, 1), jnp.where(odd, me, 3)]
    tgt = [(me + k) & 3 for k in koff]

    def xcp(r, sem):
        return pltpu.make_async_copy(x_hbm.at[pl.ds(pl.multiple_of(tgt[r] * BLK, BLK), BLK), :], x_v.at[r], sem)
    cp_idx = pltpu.make_async_copy(idx_hbm, idx_v, ld_sem.at[0])
    cp_rw = pltpu.make_async_copy(rw_hbm, rw_v, ld_sem.at[0])
    cp_x = [xcp(0, ld_sem.at[8]), xcp(1, ld_sem.at[1]), xcp(2, ld_sem.at[6]), xcp(3, ld_sem.at[7])]
    cp_sw = pltpu.make_async_copy(sw_hbm, sw_v, ld_sem.at[9])
    cp_w = [pltpu.make_async_copy(ew_hbm.at[:, :, pl.ds(c * CW, CW)], w_v.at[c], ld_sem.at[2 + c]) for c in range(NCH)]
    with scope("issue"):
        cp_idx.start()
        cp_rw.start()
        cp_x[1].start()
        pl.when(odd)(cp_x[2].start)
        for c in range(NCH):
            cp_w[c].start()
        pl.when(even)(cp_x[2].start)
        cp_x[3].start()
        cp_x[0].start()
        cp_sw.start()
        barrier = pltpu.get_barrier_semaphore()
        for r in (1, 2, 3):
            pl.semaphore_signal(barrier, inc=1, device_id=(tgt[r],), device_id_type=MESH)

    r_i = lax.broadcasted_iota(i32, (BLK, BLK), 0)
    c_i = lax.broadcasted_iota(i32, (BLK, BLK), 1)
    row = lax.broadcasted_iota(i32, (8, BLK), 0)
    lane = lax.broadcasted_iota(i32, (8, BLK), 1)

    with scope("wait_idx"):
        cp_idx.wait()
        cp_rw.wait()
    with scope("meta"):
        idx4 = idx_v[...]
        kk = row & 3
        blk = jnp.where(kk == 0, tgt[0], jnp.where(kk == 1, tgt[1], jnp.where(kk == 2, tgt[2], tgt[3])))
        e_send = jnp.zeros((8, BLK), i32)
        for d in range(NDEV):
            e_send = jnp.where(blk == d, jnp.broadcast_to(idx4[d:d + 1, :], (8, BLK)), e_send)
        e_own = jnp.broadcast_to(e_send[0:1, :], (8, BLK))
        m_send = (e_send >> 1) == me
        m_recv = (e_own >> 1) == ((me - kk) & 3)
        maskf = jnp.where(row < 4, jnp.where(m_send, 1.0, 0.0), jnp.where(m_recv, 1.0, 0.0)).astype(f32)
        upper = jnp.where(r_i < c_i, 1.0, 0.0).astype(bf16)
        m16 = jnp.concatenate([maskf, maskf], axis=0).astype(bf16)
        rank = _dot(m16, upper)[0:8, :].astype(i32)
        incl = rank + maskf.astype(i32)
        grp = (incl + (G - 1)) >> 4
        packed = jnp.sum(jnp.where(lane == BLK - 1, grp << (4 * row), 0))
        ngrp = [(packed >> (4 * r)) & 0xF for r in range(8)]

    def onehots(r, off=0):
        rk = jnp.broadcast_to(rank[r:r + 1, :], (BLK, BLK)) + off
        ek = jnp.broadcast_to(e_send[r:r + 1, :], (BLK, BLK))
        hit = rk == r_i
        p0 = jnp.where(hit & (ek == 2 * me), 1.0, 0.0).astype(bf16)
        p1 = jnp.where(hit & (ek == 2 * me + 1), 1.0, 0.0).astype(bf16)
        return p0, p1

    def compact(parts):
        ps0, ps1, xs = [], [], []
        for r, off in parts:
            p0, p1 = onehots(r, off)
            ps0.append(p0); ps1.append(p1); xs.append(x_v[r].astype(bf16))
        pm = jnp.concatenate([jnp.concatenate(ps0, axis=1), jnp.concatenate(ps1, axis=1)], axis=0)
        xc = _dot(pm, jnp.concatenate(xs, axis=0))
        return jnp.concatenate([xc[0:BLK], xc[BLK:2 * BLK]], axis=1).astype(bf16)

    def wcols(c0, n):
        return jnp.concatenate([w_v[c0 + j].astype(bf16).reshape(EL * D, CW) for j in range(n)], axis=1)

    def send(r, c, src_grp):
        n = ngrp[r]
        @pl.when(n > 0)
        def _():
            pltpu.make_async_remote_copy(
                send_v.at[pl.ds(src_grp, n), :, pl.ds(c * CW, CW)],
                recv_v.at[pl.ds((koff[r] - 1) * NG, n), :, pl.ds(c * CW, CW)],
                send_sem.at[0], recv_sem.at[c], device_id=(tgt[r],), device_id_type=MESH).start()

    def run_pass(parts, base, paced):
        lhs_v[...] = _pack(compact([(r, off) for r, off, _ in parts]))
        for c in range(NCH):
            if paced:
                with scope(f"wait_w{c}"):
                    cp_w[c].wait()
            with scope(f"mm{parts[0][0]}_{c}"):
                y = _dot(_unpack(lhs_v[...]), wcols(c, 1)).astype(bf16)
                send_v[base:base + NG, :, c * CW:(c + 1) * CW] = _pack(y)
                @pl.when(late)
                def _():
                    if paced and c == 0:
                        pl.semaphore_wait(barrier, NDEV - 1)
                    for r, _, src in parts:
                        send(r, c, src)

    def single(r, paced):
        run_pass([(r, 0, (r - 1) * NG)], (r - 1) * NG, paced)

    def pair_src(ra, rb):
        fits = ngrp[ra] + ngrp[rb] <= NG
        return fits, jnp.where(fits, (ra - 1) * NG + ngrp[ra], (rb - 1) * NG)

    def pair(ra, rb, paced):
        fits, src_b = pair_src(ra, rb)
        base = (ra - 1) * NG
        lhs_v[...] = _pack(compact([(ra, 0), (rb, jnp.where(fits, ngrp[ra] * G, BLK))]))
        for c in range(NCH):
            if paced:
                with scope(f"wait_w{c}"):
                    cp_w[c].wait()
            with scope(f"mm{ra}{rb}_{c}"):
                y = _dot(_unpack(lhs_v[...]), wcols(c, 1)).astype(bf16)
                send_v[base:base + NG, :, c * CW:(c + 1) * CW] = _pack(y)
                @pl.when(late)
                def _():
                    if paced and c == 0:
                        pl.semaphore_wait(barrier, NDEV - 1)
                    send(ra, c, base)
                    pl.when(fits)(lambda: send(rb, c, src_b))
        @pl.when(jnp.logical_not(fits))
        def _():
            single(rb, False)

    with scope("wait_x1"):
        cp_x[1].wait()
    @pl.when(odd)
    def _():
        cp_x[2].wait()
        pair(1, 2, True)
    @pl.when(even)
    def _():
        single(1, True)
        cp_x[2].wait()
    with scope("wait_x3"):
        cp_x[3].wait()
    @pl.when(odd)
    def _():
        single(3, False)
    @pl.when(even)
    def _():
        pair(2, 3, False)

    with scope("first_sends"):
        @pl.when(first)
        def _():
            _, src3 = pair_src(2, 3)
            pl.semaphore_wait(barrier, NDEV - 1)
            for c in range(NCH):
                send(1, c, 0)
                send(2, c, NG)
                send(3, c, src3)

    with scope("wait_x0"):
        cp_x[0].wait()
    with scope("router"):
        xo = x_v[0].astype(bf16)
        st = lax.dot_general(rw_v[...].astype(bf16), xo, (((1,), (1,)), ((), ())),
                             preferred_element_type=f32)
        smax = jnp.max(st, axis=0, keepdims=True)
        ex = jnp.exp(st - smax)
        probs = ex / jnp.sum(ex, axis=0, keepdims=True)
        p_sel = jnp.sum(jnp.where(row == e_own, probs, 0.0), axis=0, keepdims=True)
        pb = jnp.broadcast_to(p_sel, (BLK, BLK))
        for j in range(NDEV):
            rk = jnp.broadcast_to(rank[4 + j:5 + j, :], (BLK, BLK))
            mk = jnp.broadcast_to(maskf[4 + j:5 + j, :], (BLK, BLK))
            pk = jnp.where((rk == r_i) & (mk > 0.5), pb, 0.0)
            pt_v[:, :, j * BLK:(j + 1) * BLK] = _pack(pk.T.astype(bf16))
    with scope("own"):
        lo = compact([(0, 0)])
        own_v[...] = _pack(_dot(lo, wcols(0, NCH)).astype(bf16))
    with scope("wait_sw"):
        cp_sw.wait()
    with scope("shared"):
        lhs = jnp.concatenate([xo, _unpack(pt_v[:, :, 0:BLK])], axis=1)
        rhs = jnp.concatenate([sw_v[...].astype(bf16), _unpack(own_v[...])], axis=0)
        out_ref[...] = _dot(lhs, rhs)

    total = ngrp[5] + ngrp[6] + ngrp[7]
    gidx = lax.broadcasted_iota(i32, (3 * NG, 8, CW), 0)
    lim = jnp.where(gidx < NG, ngrp[5], jnp.where(gidx < 2 * NG, NG + ngrp[6], 2 * NG + ngrp[7]))
    valid = gidx < lim
    for (c0, c1) in STAGES:
        with scope(f"recv{c0}_{c1}"):
            for c in range(c0, c1 + 1):
                @pl.when(total > 0)
                def _():
                    buf = recv_v.at[pl.ds(0, total), :, pl.ds(c * CW, CW)]
                    pltpu.make_async_copy(buf, buf, recv_sem.at[c]).wait()
        with scope(f"acc{c0}_{c1}"):
            rls = [jnp.where(valid, recv_v[:, :, c * CW:(c + 1) * CW], jnp.uint32(0)) for c in range(c0, c1 + 1)]
            rr = _unpack(jnp.concatenate(rls, axis=2))
            out_ref[:, c0 * CW:(c1 + 1) * CW] += _dot(_unpack(pt_v[:, :, BLK:4 * BLK]), rr)
    with scope("wait_sends"):
        nsend = ngrp[1] + ngrp[2] + ngrp[3]
        @pl.when(nsend > 0)
        def _():
            buf = send_v.at[pl.ds(0, nsend)]
            pltpu.make_async_copy(buf, buf, send_sem.at[0]).wait()


def pallas_dist_moe_shared_ep_outshard_n512_d256_e2_h512_kernel(x, router_W, route_idx, expert_W, shared_W):
    any_spec = pl.BlockSpec(memory_space=pl.ANY)
    return pl.pallas_call(
        _body,
        out_shape=jax.ShapeDtypeStruct((BLK, H), f32),
        in_specs=[any_spec] * 5,
        out_specs=pl.BlockSpec(memory_space=pltpu.VMEM),
        scratch_shapes=[
            pltpu.VMEM((NDEV, BLK), i32),
            pltpu.VMEM((NE, D), f32),
            pltpu.VMEM((NDEV, BLK, D), f32),
            pltpu.VMEM((NCH, EL, D, CW), f32),
            pltpu.VMEM((D, H), f32),
            pltpu.VMEM((NG, 8, EL * D), u32),
            pltpu.VMEM((3 * NG, 8, H), u32),
            pltpu.VMEM((3 * NG, 8, H), u32),
            pltpu.VMEM((NG, 8, H), u32),
            pltpu.VMEM((NG, 8, NDEV * BLK), u32),
            pltpu.SemaphoreType.DMA((10,)),
            pltpu.SemaphoreType.DMA((1,)),
            pltpu.SemaphoreType.DMA((NCH,)),
        ],
        compiler_params=pltpu.CompilerParams(collective_id=0, disable_semaphore_checks=bool(NOSEMCHK),
                                             disable_bounds_checks=bool(NOBOUNDS)),
    )(x, router_W.T, route_idx.reshape(NDEV, BLK), expert_W, shared_W)
```

```python
import functools, contextlib
import jax
import jax.numpy as jnp
from jax import lax
from jax.experimental import pallas as pl
from jax.experimental.pallas import tpu as pltpu

NDEV = 4
NTOK = 512
BLK = NTOK // NDEV
D = 256
H = 512
NE = 8
EL = 2
NCH = 4
CW = H // NCH
G = 16
NG = BLK // G
MESH = pl.DeviceIdType.MESH
bf16, f32, i32, u32 = jnp.bfloat16, jnp.float32, jnp.int32, jnp.uint32

SCOPES = False
NOSEMCHK = 0
NOBOUNDS = 0
SMALLM = 3
EARLYPOS = 2
SMALLK = 4

def scope(name):
    return jax.named_scope(name) if SCOPES else contextlib.nullcontext()

def _dot(a, b):
    return jnp.dot(a, b, preferred_element_type=f32)

def _pack(v):
    w = pltpu.bitcast(v, u32)
    return w.reshape(w.shape[0] // 8, 8, w.shape[1])

def _unpack(w):
    return pltpu.bitcast(w.reshape(w.shape[0] * 8, w.shape[2]), bf16)


def _body(x_hbm, rw_hbm, idx_hbm, ew_hbm, sw_hbm, out_ref,
          idx_v, rw_v, x_v, w_v, sw_v, lhs_v, send_v, recv_v, own_v, pt_v,
          ld_sem, send_sem, recv_sem):
    me = lax.axis_index("i")
    odd = (me & 1) == 1
    even = jnp.logical_not(odd)
    first = me == 0
    late = jnp.logical_not(first)
    koff = [0, jnp.where(odd, (-me) & 3, 2), jnp.where(odd, 2, 1), jnp.where(odd, me, 3)]
    tgt = [(me + k) & 3 for k in koff]
    slot = [None] + [jnp.where(k == 2, 2, k >> 1) for k in koff[1:]]

    def xcp(r, sem):
        return pltpu.make_async_copy(x_hbm.at[pl.ds(pl.multiple_of(tgt[r] * BLK, BLK), BLK), :], x_v.at[r], sem)
    cp_idx = pltpu.make_async_copy(idx_hbm, idx_v, ld_sem.at[0])
    cp_rw = pltpu.make_async_copy(rw_hbm, rw_v, ld_sem.at[7])
    cp_x1 = xcp(1, ld_sem.at[1])
    cp_x2a = xcp(2, ld_sem.at[1])
    cp_x2b = xcp(2, ld_sem.at[6])
    cp_x3 = xcp(3, ld_sem.at[6])
    cp_x0 = xcp(0, ld_sem.at[7])
    cp_sw = pltpu.make_async_copy(sw_hbm, sw_v, ld_sem.at[7])
    cp_w = [pltpu.make_async_copy(ew_hbm.at[:, :, pl.ds(c * CW, CW)], w_v.at[c], ld_sem.at[2 + c]) for c in range(NCH)]
    with scope("issue"):
        cp_idx.start()
        cp_x1.start()
        pl.when(odd)(cp_x2a.start)
        for c in range(NCH):
            cp_w[c].start()
        pl.when(even)(cp_x2b.start)
        cp_x3.start()
        cp_rw.start()
        cp_x0.start()
        cp_sw.start()
        barrier = pltpu.get_barrier_semaphore()
        for r in (1, 2, 3):
            pl.semaphore_signal(barrier, inc=1, device_id=(tgt[r],), device_id_type=MESH)

    r_i = lax.broadcasted_iota(i32, (BLK, BLK), 0)
    c_i = lax.broadcasted_iota(i32, (BLK, BLK), 1)
    row = lax.broadcasted_iota(i32, (8, BLK), 0)
    lane = lax.broadcasted_iota(i32, (8, BLK), 1)

    with scope("wait_idx"):
        cp_idx.wait()
    with scope("meta"):
        idx4 = idx_v[...]
        kk = row & 3
        blk = jnp.where(kk == 0, tgt[0], jnp.where(kk == 1, tgt[1], jnp.where(kk == 2, tgt[2], tgt[3])))
        e_send = jnp.zeros((8, BLK), i32)
        for d in range(NDEV):
            e_send = jnp.where(blk == d, jnp.broadcast_to(idx4[d:d + 1, :], (8, BLK)), e_send)
        e_own = jnp.broadcast_to(e_send[0:1, :], (8, BLK))
        m_send = (e_send >> 1) == me
        back = jnp.where(kk == 2, 3, jnp.where(kk == 3, 2, kk))
        m_recv = (e_own >> 1) == ((me - back) & 3)
        maskf = jnp.where(row < 4, jnp.where(m_send, 1.0, 0.0), jnp.where(m_recv, 1.0, 0.0)).astype(f32)
        upper = jnp.where(r_i < c_i, 1.0, 0.0).astype(bf16)
        m16 = jnp.concatenate([maskf, maskf], axis=0).astype(bf16)
        rank = _dot(m16, upper)[0:8, :].astype(i32)
        incl = rank + maskf.astype(i32)
        grp = (incl + (G - 1)) >> 4
        packed = jnp.sum(jnp.where(lane == BLK - 1, grp << (4 * row), 0))
        ngrp = [(packed >> (4 * r)) & 0xF for r in range(8)]

    def onehots(r, off):
        rk = jnp.broadcast_to(rank[r:r + 1, :], (BLK, BLK)) + off
        ek = jnp.broadcast_to(e_send[r:r + 1, :], (BLK, BLK))
        hit = rk == r_i
        p0 = jnp.where(hit & (ek == 2 * me), 1.0, 0.0).astype(bf16)
        p1 = jnp.where(hit & (ek == 2 * me + 1), 1.0, 0.0).astype(bf16)
        return p0, p1

    def compact(parts):
        ps0, ps1, xs = [], [], []
        for r, off in parts:
            p0, p1 = onehots(r, off)
            ps0.append(p0); ps1.append(p1); xs.append(x_v[r].astype(bf16))
        pm = jnp.concatenate([jnp.concatenate(ps0, axis=1), jnp.concatenate(ps1, axis=1)], axis=0)
        xc = _dot(pm, jnp.concatenate(xs, axis=0))
        return jnp.concatenate([xc[0:BLK], xc[BLK:2 * BLK]], axis=1).astype(bf16)

    def wcols(c0, n):
        return jnp.concatenate([w_v[c0 + j].astype(bf16).reshape(EL * D, CW) for j in range(n)], axis=1)

    def send(r, c, src_grp):
        n = ngrp[r]
        @pl.when(n > 0)
        def _():
            sem = recv_sem.at[jnp.where(odd, NCH, c)]
            pltpu.make_async_remote_copy(
                send_v.at[c, pl.ds(src_grp, n)],
                recv_v.at[c, pl.ds(slot[r] * NG, n)],
                send_sem.at[0], sem, device_id=(tgt[r],), device_id_type=MESH).start()

    def expert_chunk(base, c, g):
        y = _dot(_unpack(lhs_v[0:g]), wcols(c, 1)).astype(bf16)
        send_v[c, base:base + g] = _pack(y)

    def single(r, paced):
        base = (r - 1) * NG
        lhs_v[...] = _pack(compact([(r, 0)]))
        for c in range(NCH):
            if paced:
                with scope(f"wait_w{c}"):
                    cp_w[c].wait()
            with scope(f"mm{r}_{c}"):
                if paced and c == NCH - 1 and SMALLM:
                    short = ngrp[r] <= SMALLM
                    pl.when(short)(lambda: expert_chunk(base, c, SMALLM))
                    pl.when(jnp.logical_not(short))(lambda: expert_chunk(base, c, NG))
                else:
                    expert_chunk(base, c, NG)
                @pl.when(late)
                def _():
                    if paced and c == 0:
                        pl.semaphore_wait(barrier, NDEV - 1)
                    send(r, c, base)

    def pair_src(ra, rb):
        fits = ngrp[ra] + ngrp[rb] <= NG
        return fits, jnp.where(fits, (ra - 1) * NG + ngrp[ra], (rb - 1) * NG)

    def pair(ra, rb, paced):
        fits, src_b = pair_src(ra, rb)
        base = (ra - 1) * NG
        lhs_v[...] = _pack(compact([(ra, 0), (rb, jnp.where(fits, ngrp[ra] * G, BLK))]))
        for c in range(NCH):
            if paced:
                with scope(f"wait_w{c}"):
                    cp_w[c].wait()
            with scope(f"mm{ra}{rb}_{c}"):
                expert_chunk(base, c, NG)
                @pl.when(late)
                def _():
                    if paced and c == 0:
                        pl.semaphore_wait(barrier, NDEV - 1)
                    send(ra, c, base)
                    pl.when(fits)(lambda: send(rb, c, src_b))
        @pl.when(jnp.logical_not(fits))
        def _():
            single(rb, False)

    @pl.when(odd)
    def _():
        with scope("wait_x12"):
            cp_x1.wait()
            cp_x2a.wait()
        pair(1, 2, True)
        with scope("wait_x3"):
            cp_x3.wait()
        single(3, False)

    @pl.when(even)
    def _():
        with scope("wait_x1"):
            cp_x1.wait()
        single(1, True)
        with scope("wait_x23"):
            cp_x2b.wait()
            cp_x3.wait()
        pair(2, 3, False)

    with scope("first_sends"):
        @pl.when(first)
        def _():
            _, src3 = pair_src(2, 3)
            pl.semaphore_wait(barrier, NDEV - 1)
            for c in range(NCH):
                send(1, c, 0)
                send(2, c, NG)
                send(3, c, src3)

    with scope("wait_x0"):
        cp_rw.wait()
        cp_x0.wait()
        cp_sw.wait()
    with scope("router"):
        xo = x_v[0].astype(bf16)
        st = lax.dot_general(rw_v[...].astype(bf16), xo, (((1,), (1,)), ((), ())),
                             preferred_element_type=f32)
        smax = jnp.max(st, axis=0, keepdims=True)
        ex = jnp.exp(st - smax)
        probs = ex / jnp.sum(ex, axis=0, keepdims=True)
        p_sel = jnp.sum(jnp.where(row == e_own, probs, 0.0), axis=0, keepdims=True)
        pb = jnp.broadcast_to(p_sel, (BLK, BLK))
        for j in range(NDEV):
            rk = jnp.broadcast_to(rank[4 + j:5 + j, :], (BLK, BLK))
            mk = jnp.broadcast_to(maskf[4 + j:5 + j, :], (BLK, BLK))
            pk = jnp.where((rk == r_i) & (mk > 0.5), pb, 0.0)
            pt_v[:, :, j * BLK:(j + 1) * BLK] = _pack(pk.T.astype(bf16))
    with scope("own"):
        lo = compact([(0, 0)])
        own_v[...] = _pack(_dot(lo, wcols(0, NCH)).astype(bf16))

    n_nbr = ngrp[5] + ngrp[6]
    n_diag = ngrp[7]

    def received(s0, ns, g, c):
        gidx = lax.broadcasted_iota(i32, (ns * g, 8, CW), 0)
        if ns == 1:
            lim = ngrp[5 + s0]
        else:
            lim = jnp.where(gidx < NG, ngrp[5 + s0], NG + ngrp[6 + s0])
        return _unpack(jnp.where(gidx < lim, recv_v[c, s0 * NG:s0 * NG + ns * g], jnp.uint32(0)))

    def received_all(s0, ns):
        return jnp.concatenate([received(s0, ns, NG, c) for c in range(NCH)], axis=1)

    def wait_recv(n, sem, cs):
        @pl.when(n > 0)
        def _():
            buf = recv_v.at[cs, pl.ds(0, n)]
            pltpu.make_async_copy(buf, buf, sem).wait()

    def first_stage(s0, ns):
        lhs = jnp.concatenate([xo, _unpack(pt_v[:, :, 0:BLK]), _unpack(pt_v[:, :, (1 + s0) * BLK:(1 + s0 + ns) * BLK])], axis=1)
        rhs = jnp.concatenate([sw_v[...].astype(bf16), _unpack(own_v[...]), received_all(s0, ns)], axis=0)
        out_ref[...] = _dot(lhs, rhs)

    MS = 4
    def late_stage(s0, ns, c, g):
        rr = received(s0, ns, g, c)
        for m in range(MS):
            rows = slice(m * (BLK // MS), (m + 1) * (BLK // MS))
            grs = slice(m * (NG // MS), (m + 1) * (NG // MS))
            pt = _unpack(pt_v[grs, :, (1 + s0) * BLK:(1 + s0) * BLK + ns * g * G])
            out_ref[rows, c * CW:(c + 1) * CW] += _dot(pt, rr)

    @pl.when(even)
    def _():
        with scope("first_stage"):
            lhs = jnp.concatenate([xo, _unpack(pt_v[:, :, 0:BLK])], axis=1)
            rhs = jnp.concatenate([sw_v[...].astype(bf16), _unpack(own_v[...])], axis=0)
            out_ref[...] = _dot(lhs, rhs)
        def diag_chunk(c):
            with scope(f"recv{c}"):
                wait_recv(n_diag, recv_sem.at[c], c)
            with scope(f"acc{c}"):
                if SMALLK:
                    short = n_diag <= SMALLK
                    pl.when(short)(lambda: late_stage(2, 1, c, SMALLK))
                    pl.when(jnp.logical_not(short))(lambda: late_stage(2, 1, c, NG))
                else:
                    late_stage(2, 1, c, NG)
        for c in range(EARLYPOS):
            diag_chunk(c)
        with scope("recv_early"):
            wait_recv(n_nbr, recv_sem.at[NCH], slice(None))
        with scope("early_stage"):
            out_ref[...] += _dot(_unpack(pt_v[:, :, BLK:3 * BLK]), received_all(0, 2))
        for c in range(EARLYPOS, NCH):
            diag_chunk(c)

    @pl.when(odd)
    def _():
        with scope("recv_early"):
            wait_recv(n_diag, recv_sem.at[NCH], slice(None))
        with scope("first_stage"):
            first_stage(2, 1)
        for c in range(NCH):
            with scope(f"recv{c}"):
                wait_recv(n_nbr, recv_sem.at[c], c)
            with scope(f"acc{c}"):
                late_stage(0, 2, c, NG)

    with scope("wait_sends"):
        nsend = ngrp[1] + ngrp[2] + ngrp[3]
        @pl.when(nsend > 0)
        def _():
            buf = send_v.at[:, pl.ds(0, nsend)]
            pltpu.make_async_copy(buf, buf, send_sem.at[0]).wait()


def _scoped_body(*refs):
    pl.run_scoped(
        functools.partial(_body, *refs),
        pltpu.SemaphoreType.DMA((8,)),
        pltpu.SemaphoreType.DMA((1,)),
        pltpu.SemaphoreType.DMA((NCH + 1,)),
    )


def pallas_dist_moe_shared_ep_outshard_n512_d256_e2_h512_kernel(x, router_W, route_idx, expert_W, shared_W):
    any_spec = pl.BlockSpec(memory_space=pl.ANY)
    return pl.pallas_call(
        _scoped_body,
        out_shape=jax.ShapeDtypeStruct((BLK, H), f32),
        in_specs=[any_spec] * 5,
        out_specs=pl.BlockSpec(memory_space=pltpu.VMEM),
        scratch_shapes=[
            pltpu.VMEM((NDEV, BLK), i32),
            pltpu.VMEM((NE, D), f32),
            pltpu.VMEM((NDEV, BLK, D), f32),
            pltpu.VMEM((NCH, EL, D, CW), f32),
            pltpu.VMEM((D, H), f32),
            pltpu.VMEM((NG, 8, EL * D), u32),
            pltpu.VMEM((NCH, 3 * NG, 8, CW), u32),
            pltpu.VMEM((NCH, 3 * NG, 8, CW), u32),
            pltpu.VMEM((NG, 8, H), u32),
            pltpu.VMEM((NG, 8, NDEV * BLK), u32),
        ],
        compiler_params=pltpu.CompilerParams(collective_id=0, disable_semaphore_checks=bool(NOSEMCHK),
                                             disable_bounds_checks=bool(NOBOUNDS)),
    )(x, router_W.T, route_idx.reshape(NDEV, BLK), expert_W, shared_W)
```
